```python
import numpy as np

kernel_name = "dist_moe_cap_ep_tokshard_n2048_d512_e8_h1024"

def setup_inputs():
    x = np.random.randn(8192, 512).astype(np.float32)
    router_W = np.random.randn(512, 32).astype(np.float32) * 0.1
    scores64 = x.astype(np.float64) @ router_W.astype(np.float64)
    route_idx = np.argsort(-scores64, axis=-1)[:, :1].astype(np.int32)
    expert_W = np.random.randn(32, 512, 1024).astype(np.float32) * 0.02
    return {"x": x, "router_W": router_W, "route_idx": route_idx, "expert_W": expert_W}

def reference(x, router_W, route_idx, expert_W):
    counts = np.zeros(32, dtype=np.int64)
    out = np.zeros((8192, 1024), dtype=np.float32)
    for i in range(8192):
        e = int(route_idx[i, 0])
        if counts[e] < 204:
            out[i] = x[i] @ expert_W[e]
            counts[e] += 1
    return out
```

```python
import jax
import jax.numpy as jnp
from jax import lax
from jax.experimental import pallas as pl
from jax.experimental.pallas import tpu as pltpu

T = 2048
D = 512
H = 1024
NE = 32
EL = 8
CAP = 204
NB = 8
BT = T // NB
NC = NB * NE

LX = 4
LY = 4
CX, CY = 1 << LX, 1 << LY
NRX = 352 >> LX
NRY = 640 >> LY
NBITS = 11
NSX, NSY = NRX + NBITS, NRY + NBITS
XS = (LX, NRX)
YS = (LY, NRY)
XP = 16
HX = T // 2 + XP
RX = 2 * HX
RY = 1664
DUMMYX = XP + 7 * RX
ZEROY = 8 * RY
MT = 128
BIG = 1 << 20

K1OFF = 13
ES = 4
CN_POS = 1
C3_POS = 4
FWD_BIAS = 120
LEAD = 2
DRAIN_B = 5

U32 = jnp.uint32
I32 = jnp.int32
F32 = jnp.float32
BF16 = jnp.bfloat16
MESH = pl.DeviceIdType.MESH


def _task_key(g, e):
    return 4 * e if g == 0 else max(4 * e + 1, 2 * e + K1OFF)


_TASKS = sorted([(g, e) for g in range(2) for e in range(EL)],
                key=lambda t: (_task_key(*t), t[0]))
assert all(g == 0 for g, _ in _TASKS[:max(CN_POS, C3_POS)])

ST_XA = 0
ST_XIN = 8
ST_XOUT = 16
ST_XS = 24
ST_YS = 32
ST_YA = 36
ST_YIN = 40
ST_YOUT = 44
ST_F0 = 48
ST_F1 = 49
ST_LD = 50
ST_TG = 56
ST_TE = 72
ST_N = 88


def _pack2(a, b):
    lo = lax.bitcast_convert_type(a.astype(BF16).astype(F32), U32) >> 16
    hi = lax.bitcast_convert_type(b.astype(BF16).astype(F32), U32)
    return hi | lo


def _unlo(w):
    return lax.bitcast_convert_type(w << 16, F32)


def _unhi(w):
    return lax.bitcast_convert_type(w & jnp.uint32(0xFFFF0000), F32)


def _dot(a, b):
    return jnp.dot(a, b, preferred_element_type=F32)


def _dot_nt(a, b):
    return lax.dot_general(a, b, (((1,), (1,)), ((), ())),
                           preferred_element_type=F32)


def _onez(mask):
    return jnp.where(mask, 1.0, 0.0).astype(BF16)


def _body(x_hbm, route_hbm, w_hbm, out_ref,
          xv, wv, rv, xtok, xb, yb, stg, ystg, ytok,
          oh, rk, cnt, cm, tabv, earlyv, fastv,
          tabs, earlys, fasts, st,
          sem_l, sem_cs, sem_cr,
          sem_xs, sem_xr, sem_ys, sem_yr, sem_fs, sem_fr):
    me = lax.axis_index("i")

    route_cp = pltpu.make_async_copy(route_hbm, rv, sem_l.at[0])
    route_cp.start()

    def x_cp(p):
        return pltpu.make_async_copy(x_hbm.at[pl.ds(p * BT, BT)],
                                     xv.at[pl.ds(p * BT, BT)], sem_l.at[5 + p])

    def w_cp(e):
        return pltpu.make_async_copy(w_hbm.at[e], wv.at[e], sem_l.at[13 + e])

    for p in range(4):
        x_cp(p).start()

    bar = pltpu.get_barrier_semaphore()
    for k in range(1, 4):
        pl.semaphore_signal(bar, inc=1, device_id=((me + k) & 3,),
                            device_id_type=MESH)

    def rest_loads(pos):
        for e in range(EL):
            if e == pos:
                for p in range(4, NB):
                    x_cp(p).start()
            w_cp(e).start()

    @pl.when(me == 3)
    def _():
        rest_loads(C3_POS)

    @pl.when(me < 3)
    def _():
        rest_loads(CN_POS)

    def iota2(dim):
        return lax.broadcasted_iota(I32, (NC, NC), dim)

    def xkey(c):
        b = c >> 5
        xg = jnp.where(b == 0, 0, 32)
        return (((c & 31) >> 3) * 2 + (b >> 2)) * 64 + xg + (c & 7) * 4 + (b & 3)

    def ykey(c):
        b = c >> 5
        e = c & 7
        g = c >> 7
        k0 = 8 * e
        k1 = jnp.maximum(8 * e + 2, 4 * e + 2 * K1OFF) + 1
        kt = jnp.where(g == 0, k0, k1) * 4 + (b & 3)
        kp = 1024 + b * 8 + e
        kk = jnp.where((g == 1) & (e >= ES), kp, kt)
        return ((c & 31) >> 3) * 2048 + kk

    cm[1] = _onez(iota2(0) < iota2(1))
    kxi, kxj = xkey(iota2(0)), xkey(iota2(1))
    cm[0] = _onez((kxi < kxj) & (kxi >= (kxj & ~63)))

    r8 = lax.broadcasted_iota(I32, (8, NC), 0)
    c8 = lax.broadcasted_iota(I32, (8, NC), 1)
    blk8 = (c8 >> 5) == r8
    krel8 = (((c8 & 31) >> 3) - me) & 3

    for i in range(ST_TG):
        st[i] = 0
    for i, (g, e) in enumerate(_TASKS):
        st[ST_TG + i] = g
        st[ST_TE + i] = e

    route_cp.wait()
    fast_cp = pltpu.make_async_copy(fastv, fasts, sem_l.at[4])

    @pl.when(me < 3)
    def _():
        e128 = lax.broadcasted_iota(I32, (128, 128), 0)
        oh0 = jnp.concatenate(
            [_onez(e128 == rv[h:h + 1, :]) for h in range(2)], axis=1)
        raw0 = _dot_nt(jnp.ones((8, BT), BF16), oh0)
        pre0 = _dot(oh0[0:NE], cm[1])
        rank0 = jnp.sum(oh0[0:NE].astype(F32) * pre0, axis=0, keepdims=True)
        off0 = _dot(raw0.astype(BF16), cm[0, 0:128, 0:128]).astype(I32)
        v0 = off0 + krel8[:, :128] * RX + XP
        r0 = r8[:, :128]
        l0 = jnp.where(r0 == 0, v0 >> 7, v0 & 127)
        l0 = jnp.concatenate([l0, l0], axis=0).astype(F32).astype(BF16)
        lk0 = _dot(l0, oh0)
        pos0 = (lk0[0:1] * 128.0 + lk0[1:2] + rank0).astype(I32) * 2
        end0 = off0 + raw0.astype(I32)
        fastv[...] = jnp.where(r0 == 0, pos0[:, :128],
                               jnp.where(r0 == 1, pos0[:, 128:], end0))
        fast_cp.start()

    e32 = lax.broadcasted_iota(I32, (NE, 128), 0)
    for b in range(NB):
        for h in range(2):
            rb = rv[2 * b + h:2 * b + h + 1, :]
            oh[b * NE:(b + 1) * NE, 128 * h:128 * h + 128] = _onez(e32 == rb)
    ohv = oh[...]
    raw = _dot_nt(jnp.ones((8, BT), BF16), ohv)
    cnt[me] = raw

    def cnt_cp(k):
        return pltpu.make_async_remote_copy(
            src_ref=cnt.at[me], dst_ref=cnt.at[me],
            send_sem=sem_cs.at[k - 1], recv_sem=sem_cr.at[k - 1],
            device_id=((me + k) & 3,), device_id_type=MESH)

    pl.semaphore_wait(bar, 3)
    for k in range(1, 4):
        cnt_cp(k).start()

    def pack_block(p):
        x_cp(p).wait()
        for h in range(2):
            r0 = pl.multiple_of(p * BT + h * 128, 128)
            xf = xv[pl.ds(r0, 128), :]
            xtok[pl.ds(2 * r0, 128, stride=2), :] = _pack2(
                xf[:, 0:128], xf[:, 128:256])
            xtok[pl.ds(2 * r0 + 1, 128, stride=2), :] = _pack2(
                xf[:, 256:384], xf[:, 384:512])

    def scatter_rows(pos_ref, lo, hi):
        def loop(r, _):
            base = r * 256
            for u in range(128):
                qq = pos_ref[r, u]
                xb[pl.ds(qq, 2), :] = xtok[pl.ds(base + 2 * u, 2), :]
            return 0
        lax.fori_loop(lo, hi, loop, 0)

    def x_copy_h(hf):
        def x_copy(k, off, n, sidx):
            o = XP + hf * HX + off
            return pltpu.make_async_remote_copy(
                src_ref=xb.at[pl.ds(2 * (k * RX + o), 2 * n)],
                dst_ref=xb.at[pl.ds(2 * ((3 + k) * RX + o), 2 * n)],
                send_sem=sem_xs.at[k - 1],
                recv_sem=sem_xr.at[(3 * hf + k - 1) * NSX + sidx],
                device_id=((me + k) & 3,), device_id_type=MESH)
        return x_copy

    def y_copy(k, off, n, sidx):
        return pltpu.make_async_remote_copy(
            src_ref=yb.at[pl.ds(4 * (k * RY + off), 4 * n)],
            dst_ref=yb.at[pl.ds(4 * ((3 + k) * RY + off), 4 * n)],
            send_sem=sem_ys.at[k - 1], recv_sem=sem_yr.at[(k - 1) * NSY + sidx],
            device_id=((me - k) & 3,), device_id_type=MESH)

    def y_to_relay(c):
        return pltpu.make_async_remote_copy(
            src_ref=yb.at[pl.ds(4 * (2 * RY + c * CY), 4 * CY)],
            dst_ref=yb.at[pl.ds(4 * (7 * RY + c * CY), 4 * CY)],
            send_sem=sem_ys.at[1], recv_sem=sem_fr.at[c],
            device_id=(me ^ 1,), device_id_type=MESH)

    def y_from_relay(c):
        return pltpu.make_async_remote_copy(
            src_ref=yb.at[pl.ds(4 * (7 * RY + c * CY), 4 * CY)],
            dst_ref=yb.at[pl.ds(4 * (5 * RY + c * CY), 4 * CY)],
            send_sem=sem_fs, recv_sem=sem_yr.at[NSY + c],
            device_id=(me ^ 3,), device_id_type=MESH)

    def nfull(cfg, n):
        return jnp.minimum(n >> cfg[0], cfg[1])

    def branch(cond, fn):
        def f(i, _):
            fn()
            return 0
        lax.fori_loop(0, cond.astype(I32), f, 0)

    def tail_pieces(copy, cfg, k, n, fn):
        lc, nreg = cfg
        base = nfull(cfg, n) << lc
        r = n - base

        def bits(lo, hi):
            for bit in range(hi - 1, lo - 1, -1):
                @pl.when(((r >> bit) & 1) == 1)
                def _():
                    off = base + ((r >> (bit + 1)) << (bit + 1))
                    fn(copy(k, off, 1 << bit, nreg + bit))

        branch(r >= (1 << lc), lambda: bits(lc, NBITS))
        bits(0, lc)

    def start_(c):
        c.start()

    def wait_recv_(c):
        c.wait_recv()

    def wait_send_(c):
        c.wait_send()

    def ensure(copy, cfg, k, upto, i_a, i_len):
        lc, nreg = cfg
        have = st[i_a + k]
        n = st[i_len + k]
        nf = nfull(cfg, n)
        need = jnp.minimum((upto + ((1 << lc) - 1)) >> lc, nf)
        hc = have >> lc
        for j in range(3):
            @pl.when(hc + j < need)
            def _():
                copy(k, (hc + j) << lc, 1 << lc, hc + j).wait_recv()
        in_tail = (upto > (nf << lc)) & (have < BIG)
        st[i_a + k] = jnp.where(in_tail, BIG, jnp.maximum(have, need << lc))

        def rest():
            def loop(c, _):
                copy(k, c << lc, 1 << lc, c).wait_recv()
                return 0
            lax.fori_loop(hc + 3, need, loop, 0)
            branch(in_tail, lambda: tail_pieces(copy, cfg, k, n, wait_recv_))
        branch((need > hc + 3) | in_tail, rest)

    def send_upto(send_chunk, cfg, i_s, wm, kdir):
        s0 = [st[i_s + k] for k in range(1, 4)]
        tgt = [jnp.maximum(s0[k - 1], nfull(cfg, wm[k - 1])) for k in range(1, 4)]
        cn = [tgt[i] - s0[i] for i in range(3)]
        cntmax = jnp.maximum(jnp.maximum(cn[0], cn[1]), cn[2])
        ld = st[ST_LD]

        def loop(i, _):
            for k in (2, 1, 3):
                j = i if k == 2 else i + ld

                @pl.when((j >= 0) & (j < cn[k - 1]))
                def _():
                    send_chunk(k, s0[k - 1] + j)
            return 0
        lax.fori_loop(-ld, cntmax, loop, 0)
        for k in range(1, 4):
            st[i_s + k] = tgt[k - 1]
        na = jnp.where(kdir == 1, cn[0], cn[2])
        nd = cn[1]
        last_d = (nd > na - ld).astype(I32)
        st[ST_LD] = jnp.where(na + nd > 0, jnp.where(nd > 0, last_d, 0), ld)

    def send_y_chunk(k, c):
        if k == 2:
            relay = (c >= st[ST_F0]) & (c < st[ST_F1])

            @pl.when(relay)
            def _():
                y_to_relay(c).start()

            @pl.when(jnp.logical_not(relay))
            def _():
                y_copy(k, c * CY, CY, c).start()
        else:
            y_copy(k, c * CY, CY, c).start()

    def send_x_upto(hf, wm):
        def send_x_chunk(k, c):
            x_copy_h(hf)(k, c * CX, CX, c).start()
        send_upto(send_x_chunk, XS, ST_XS + 4 * hf, wm, 3 - 2 * (me & 1))

    def send_x_all(hf, lens):
        send_x_upto(hf, lens)
        for k in (2, 1, 3):
            tail_pieces(x_copy_h(hf), XS, k, lens[k - 1], start_)

    def send_y_upto(wm):
        send_upto(send_y_chunk, YS, ST_YS, wm, 1 + 2 * (me & 1))

    pack_block(0)

    @pl.when(me < 3)
    def _():
        fast_cp.wait()
        scatter_rows(fasts, 0, 2)
        send_x_upto(0, [fasts[2, 8 * ((me + k) & 3) + 7] for k in range(1, 4)])

    pre = _dot(ohv, cm[1])
    rank = _dot(_onez(blk8), (ohv.astype(F32) * pre).astype(BF16))
    rk[...] = rank

    def q(vi):
        return jnp.where(blk8, vi, 0).astype(F32).astype(BF16)

    early_cp = pltpu.make_async_copy(earlyv, earlys, sem_l.at[1])
    tab_cp = pltpu.make_async_copy(tabv.at[pl.ds(0, 48)], tabs.at[pl.ds(0, 48)],
                                   sem_l.at[2])
    py_cp = pltpu.make_async_copy(tabv.at[pl.ds(48, 16)], tabs.at[pl.ds(48, 16)],
                                  sem_l.at[3])

    def put_early(pos2, xend_rows):
        ev = jnp.where(r8 < 4, pos2, xend_rows)
        earlyv[pl.ds(0, 8, stride=2), :] = ev[:, :128]
        earlyv[pl.ds(1, 8, stride=2), :] = ev[:, 128:]
        early_cp.start()

    @pl.when(me < 3)
    def _():
        xoff_e = _dot(raw.astype(BF16), cm[0]).astype(I32)
        v = xoff_e + krel8 * RX + XP
        lk = _dot(jnp.concatenate([q(v >> 7), q(v & 127)], axis=0), ohv)
        pos_e = (lk[0:8] * 128.0 + lk[8:16] + rank).astype(I32) * 2
        put_early(pos_e, xoff_e + raw.astype(I32))

    def late(with_early):
        ci, cj = iota2(0), iota2(1)
        same_e = (ci & 31) == (cj & 31)
        m_e = _onez(same_e)
        m_b = _onez(same_e & (ci < cj))
        m_g = _onez(same_e & ((ci >> 7) == (cj >> 7)))
        kyi, kyj = ykey(ci), ykey(cj)
        o_y = _onez((kyi < kyj) & (kyi >= (kyj & ~2047)))

        for k in range(1, 4):
            cnt_cp(k).wait_recv()

        r16 = lax.broadcasted_iota(I32, (16, NC), 0)
        c16 = lax.broadcasted_iota(I32, (16, NC), 1)
        chip = jnp.where(r16 < 8, r16 & 3, me)
        cs = [cnt[s] for s in range(4)]
        tab = jnp.zeros((16, NC), F32)
        for s in range(4):
            tab = jnp.where(chip == s, jnp.concatenate([cs[s], cs[s]], axis=0), tab)
        tot = _dot(jnp.concatenate(cs[:3] + [cs[0]], axis=0).astype(BF16), m_e)
        cum = _dot(tab.astype(BF16), m_b)
        for s in range(3):
            ts = tot[8 * s:8 * s + 8]
            cum = cum + jnp.where(chip > s, jnp.concatenate([ts, ts], axis=0), 0.0)
        kept = jnp.clip(float(CAP) - cum, 0.0, tab)
        xc = jnp.where((chip < 3) & (c16 < 128), tab, kept)
        keptb = kept.astype(BF16)
        xoff = _dot(xc.astype(BF16), cm[0]).astype(I32)
        yoff = _dot(keptb, o_y).astype(I32)
        seg = _dot(keptb, m_g).astype(I32)
        kept_i = kept.astype(I32)
        xend = xoff + xc.astype(I32)
        vx = xoff[8:16] + krel8 * RX + (c8 >> 7) * HX + XP
        vy = yoff[8:16] + jnp.where(krel8 == 0, 0, 3 + krel8) * RY
        lhs = jnp.concatenate(
            [q(vx >> 7), q(vx & 127), q(xc[8:16].astype(I32)),
             q(vy >> 7), q(vy & 127), q(kept_i[8:16])], axis=0)
        lk = _dot(lhs, oh[...])
        rnk = rk[...]
        px = jnp.where(rnk < lk[16:24], lk[0:8] * 128.0 + lk[8:16] + rnk,
                       float(DUMMYX))
        py = jnp.where(rnk < lk[40:48], lk[24:32] * 128.0 + lk[32:40] + rnk,
                       float(ZEROY))
        pxi = px.astype(I32) * 2
        pyi = py.astype(I32) * 4
        if with_early:
            put_early(pxi, xend[8:16])

        def put(row, val):
            tabv[row:row + 8, :] = val[:, :128]
            tabv[row + 8:row + 16, :] = val[:, 128:]

        put(16, jnp.where(r8 < 4, xoff[0:8],
                          jnp.where((c8 & 127) < 32, seg[0:8], xend[0:8])))
        put(32, jnp.where(r8 < 4, yoff[0:8], kept_i[0:8]))
        for h in range(2):
            tabv[pl.ds(h, 8, stride=2), :] = pxi[:, 128 * h:128 * h + 128]
            tabv[pl.ds(48 + h, 8, stride=2), :] = pyi[:, 128 * h:128 * h + 128]
        tab_cp.start()
        py_cp.start()

    @pl.when(me == 3)
    def _():
        late(True)

    pack_block(1)
    early_cp.wait()

    def first_half(p, _):
        @pl.when(p > 1)
        def _():
            pack_block(p)
        scatter_rows(earlys, 2 * p, 2 * p + 2)

        @pl.when(p == 0)
        def _():
            send_x_upto(0, [earlys[8, 8 * ((me + k) & 3) + 7]
                            for k in range(1, 4)])
        return 0
    lax.fori_loop(jnp.where(me < 3, 1, 0), 4, first_half, 0)
    send_x_all(0, [earlys[8, 96 + 8 * ((me + k) & 3) + 7] for k in range(1, 4)])

    @pl.when(me < 3)
    def _():
        late(False)

    stg[...] = jnp.zeros(stg.shape, U32)
    yb[pl.ds(4 * ZEROY, 8), :] = jnp.zeros((8, 128), U32)

    tab_cp.wait()

    def XOFF(s, g, c):
        return tabs[16 + 8 * g + s, c]

    def SEG(s, g, c):
        return tabs[20 + 8 * g + s, c]

    def YOFF(s, g, c):
        return tabs[32 + 8 * g + s, c]

    def KEPT(s, g, c):
        return tabs[36 + 8 * g + s, c]

    def xlen_h(s, d, hf):
        return SEG(s, hf, 96 + 8 * d + 7)

    def ylen(d, s):
        c = 96 + 8 * d + 7
        return YOFF(s, 1, c) + KEPT(s, 1, c)

    for k in range(1, 4):
        for hf in range(2):
            st[ST_XIN + 4 * hf + k] = xlen_h((me - k) & 3, me, hf)
            st[ST_XOUT + 4 * hf + k] = xlen_h(me, (me + k) & 3, hf)
        st[ST_YIN + k] = ylen((me + k) & 3, me)
        st[ST_YOUT + k] = ylen(me, (me - k) & 3)

    def second_half():
        def blk(p, _):
            pack_block(p)
            scatter_rows(tabs, 2 * p, 2 * p + 2)
            return 0
        lax.fori_loop(4, NB, blk, 0)
        send_x_all(1, [st[ST_XOUT + 4 + k] for k in range(1, 4)])


    def tr(a, b):
        return xlen_h(a, b, 0) + xlen_h(a, b, 1) + 2 * ylen(a, b)

    def l3(a):
        return tr(a, a ^ 3) + tr(a, a ^ 2)

    def l1(a):
        return tr(a, a ^ 1) + tr(a ^ 3, a ^ 1)

    def relay_range(d):
        over = (jnp.maximum(l3(d), l1(d ^ 3)) - jnp.maximum(l1(d), l3(d ^ 1))
                - FWD_BIAS)
        r = jnp.maximum(over + 2 * CY, 0) >> (LY + 2)
        f1 = nfull(YS, YOFF(d ^ 2, 1, 8 * d + ES))
        return jnp.maximum(f1 - r, 0), f1

    f0, f1 = relay_range(me)
    st[ST_F0] = f0
    st[ST_F1] = f1
    p0, p1 = relay_range(me ^ 1)

    def copy_x(jobs):
        over = None
        for (src, dst, nr, nbig) in reversed(jobs):
            low = jnp.minimum(nr - 32, 0)
            for i in range(nbig):
                o = jnp.maximum(nr - 32 * (i + 1), low) if i else nr - 32
                stg[pl.ds(32 + dst + o, 32), :] = xb[pl.ds(src + o, 32), :]
            o = nr > 32 * nbig
            over = o if over is None else (over | o)

        def rest():
            for (src, dst, nr, nbig) in jobs:
                def f(i, _):
                    o = jnp.maximum(nr - 32 * (i + 1), 0)
                    stg[pl.ds(32 + dst + o, 32), :] = xb[pl.ds(src + o, 32), :]
                    return 0
                lax.fori_loop(nbig, (nr + 31) >> 5, f, 0)
        branch(over, rest)

    i32r = lax.broadcasted_iota(I32, (32, 128), 0)

    def copy_y(jobs):
        over = None
        for (src, dst, nr, nbig) in jobs:
            yb[pl.ds(dst, 32), :] = jnp.where(
                i32r < nr, ystg[pl.ds(src, 32), :], yb[pl.ds(dst, 32), :])
            ok = nr > 32
            s_ = jnp.where(ok, src, 0)
            d_ = jnp.where(ok, dst, 4 * ZEROY + 8)
            lim = jnp.maximum(nr - 32, 0)
            for i in range(1, nbig):
                o = jnp.minimum(32 * i, lim)
                yb[pl.ds(d_ + o, 32), :] = ystg[pl.ds(s_ + o, 32), :]
            o = nr > 32 * nbig
            over = o if over is None else (over | o)

        def rest():
            for (src, dst, nr, nbig) in jobs:
                def f(i, _):
                    o = jnp.minimum(i * 32, nr - 32)
                    yb[pl.ds(dst + o, 32), :] = ystg[pl.ds(src + o, 32), :]
                    return 0
                lax.fori_loop(nbig, (nr + 31) >> 5, f, 0)
        branch(over, rest)

    def task(ti, _):
        g = st[ST_TG + ti]
        e = st[ST_TE + ti]
        ee = 8 * me + e

        @pl.when(ti == jnp.where(me == 3, C3_POS, CN_POS))
        def _():
            second_half()

        @pl.when(g == 0)
        def _():
            w_cp(e).wait()

        segs = []
        xjobs = []
        row = jnp.int32(0)
        for k in range(4):
            s = (me - k) & 3
            reg = 0 if k == 0 else 3 + k
            n = SEG(s, g, ee)
            na = jnp.where(g == 0, KEPT(s, 0, ee), 0)
            nb = n - na
            sb = XOFF(s, g, ee + jnp.where(g == 0, 32, 0))
            sa = jnp.where(g == 0, XOFF(s, 0, ee), 0)
            if k > 0:
                ensure(x_copy_h(g), XS, k, sb + nb, ST_XA + 4 * g, ST_XIN + 4 * g)
            base = XP + reg * RX + g * HX
            xjobs.append((2 * (base + sa), 2 * row, 2 * na, 1))
            xjobs.append((2 * (base + sb), 2 * (row + na), 2 * nb, 3))
            segs.append((k, s, n, row))
            row = row + n
        copy_x(xjobs)

        def tile(t, _):
            r0 = t * MT
            w0 = stg[pl.ds(32 + 2 * r0, MT, stride=2), :]
            w1 = stg[pl.ds(33 + 2 * r0, MT, stride=2), :]
            lhs = jnp.concatenate(
                [_unlo(w0).astype(BF16), _unhi(w0).astype(BF16),
                 _unlo(w1).astype(BF16), _unhi(w1).astype(BF16)], axis=1)
            for j in range(4):
                wj = wv[e, :, 256 * j:256 * (j + 1)].astype(BF16)
                y = _dot(lhs, wj)
                ystg[pl.ds(4 * r0 + j, MT, stride=4), :] = _pack2(
                    y[:, :128], y[:, 128:])
            return 0
        lax.fori_loop(0, (row + (MT - 1)) >> 7, tile, 0)

        ph2 = (g == 1) & (e >= ES)

        @pl.when(jnp.logical_not(ph2))
        def _():
            copy_y([(4 * r, 4 * (k * RY + YOFF(s, g, ee)), 4 * n, 6)
                    for (k, s, n, r) in segs])
            send_y_upto([YOFF(s, g, ee) + n for (k, s, n, r) in segs[1:]])

        @pl.when(ph2)
        def _():
            jobs = []
            for (k, s, n, r) in segs:
                rr = r
                for bb in range(4):
                    cb = ee + 32 * bb
                    nb = KEPT(s, 1, cb)
                    jobs.append((4 * rr, 4 * (k * RY + YOFF(s, 1, cb)), 4 * nb, 2))
                    rr = rr + nb
            copy_y(jobs)

        return 0

    lax.fori_loop(0, 2 * EL, task, 0)


    def relay_loop(c, _):
        y_to_relay(c).wait_recv()
        y_from_relay(c).start()
        return 0
    lax.fori_loop(p0, p1, relay_loop, 0)

    pre2 = [st[ST_YS + k] for k in range(1, 4)]
    rem = [nfull(YS, st[ST_YOUT + k]) - pre2[k - 1] for k in range(1, 4)]
    fin = jnp.maximum(jnp.maximum(rem[0], rem[1]), rem[2]) + LEAD
    shift = [jnp.where((me >= 2) & (me - k == 1), LEAD, 0) for k in range(1, 4)]

    def final_loop(i, _):
        for k in (2, 1, 3):
            j = i - shift[k - 1]

            @pl.when((j >= 0) & (j < rem[k - 1]))
            def _():
                y_copy(k, (pre2[k - 1] + j) * CY, CY, pre2[k - 1] + j).start()

            @pl.when(j == rem[k - 1])
            def _():
                tail_pieces(y_copy, YS, k, st[ST_YOUT + k], start_)
        return 0
    lax.fori_loop(0, fin + 1, final_loop, 0)

    for hf in range(2):
        for k in range(1, 4):
            ensure(x_copy_h(hf), XS, k, st[ST_XIN + 4 * hf + k],
                   ST_XA + 4 * hf, ST_XIN + 4 * hf)

    def drain_send(copy, cfg, k, lo, hi):
        def loop(c, _):
            copy(k, c << cfg[0], 1 << cfg[0], c).wait_send()
            return 0
        lax.fori_loop(lo, hi, loop, 0)

    for k in range(1, 4):
        cnt_cp(k).wait_send()
        for hf in range(2):
            n = st[ST_XOUT + 4 * hf + k]
            drain_send(x_copy_h(hf), XS, k, 0, nfull(XS, n))
            tail_pieces(x_copy_h(hf), XS, k, n, wait_send_)
    py_cp.wait()

    def relay_drain(c, _):
        y_from_relay(c).wait_send()
        return 0

    def out_block(b, _):

        @pl.when(b == DRAIN_B)
        def _():
            for k in range(1, 4):
                drain_send(y_copy, YS, k, 0, pre2[k - 1])
            lax.fori_loop(p0, p1, relay_drain, 0)

        @pl.when(b == NB - 1)
        def _():
            for k in range(1, 4):
                drain_send(y_copy, YS, k, pre2[k - 1], nfull(YS, st[ST_YOUT + k]))
                tail_pieces(y_copy, YS, k, st[ST_YOUT + k], wait_send_)

        for k in range(1, 4):
            c = (b & 3) * 32 + 8 * ((me + k) & 3) + 7
            ensure(y_copy, YS, k, YOFF(me, b >> 2, c) + KEPT(me, b >> 2, c),
                   ST_YA, ST_YIN)

        def gat(h, _):
            r = 48 + 2 * b + h
            base = h * 512
            for u in range(128):
                p = tabs[r, u]
                ytok[pl.ds(base + 4 * u, 4), :] = yb[pl.ds(p, 4), :]
            return 0
        lax.fori_loop(0, 2, gat, 0)

        def unp(i, _):
            r0 = pl.multiple_of(b * BT + i * 64, 64)
            for j in range(4):
                w = ytok[pl.ds(i * 256 + j, 64, stride=4), :]
                out_ref[pl.ds(r0, 64), 256 * j:256 * j + 128] = _unlo(w)
                out_ref[pl.ds(r0, 64), 256 * j + 128:256 * j + 256] = _unhi(w)
            return 0
        lax.fori_loop(0, BT // 64, unp, 0)
        return 0

    lax.fori_loop(0, NB, out_block, 0)


def pallas_dist_moe_cap_ep_tokshard_n2048_d512_e8_h1024_kernel(
    x: jax.Array,
    router_W: jax.Array,
    route_idx: jax.Array,
    expert_W: jax.Array,
):
    del router_W
    route = route_idx.astype(I32).reshape(T // 128, 128)
    any_spec = pl.BlockSpec(memory_space=pl.ANY)
    dma = pltpu.SemaphoreType.DMA
    return pl.pallas_call(
        _body,
        out_shape=jax.ShapeDtypeStruct((T, H), F32),
        in_specs=[any_spec, any_spec, any_spec],
        out_specs=pl.BlockSpec(memory_space=pltpu.VMEM),
        scratch_shapes=[
            pltpu.VMEM((T, D), F32),
            pltpu.VMEM((EL, D, H), F32),
            pltpu.VMEM((T // 128, 128), I32),
            pltpu.VMEM((2 * T, 128), U32),
            pltpu.VMEM((2 * (DUMMYX + 4), 128), U32),
            pltpu.VMEM((4 * (ZEROY + 10), 128), U32),
            pltpu.VMEM((4 * MT + 32, 128), U32),
            pltpu.VMEM((8 * MT, 128), U32),
            pltpu.VMEM((4 * BT, 128), U32),
            pltpu.VMEM((NC, BT), BF16),
            pltpu.VMEM((8, BT), F32),
            pltpu.VMEM((4, 8, NC), F32),
            pltpu.VMEM((2, NC, NC), BF16),
            pltpu.VMEM((64, 128), I32),
            pltpu.VMEM((16, 128), I32),
            pltpu.VMEM((8, 128), I32),
            pltpu.SMEM((64, 128), I32),
            pltpu.SMEM((16, 128), I32),
            pltpu.SMEM((8, 128), I32),
            pltpu.SMEM((ST_N,), I32),
            dma((21,)), dma((3,)), dma((3,)),
            dma((3,)), dma((6 * NSX,)), dma((3,)), dma((3 * NSY,)),
            dma, dma((NRY,)),
        ],
        compiler_params=pltpu.CompilerParams(
            collective_id=0, vmem_limit_bytes=88 * 1024 * 1024,
            disable_semaphore_checks=True, disable_bounds_checks=True),
    )(x, route, expert_W)
```

```python
import jax
import jax.numpy as jnp
from jax import lax
from jax.experimental import pallas as pl
from jax.experimental.pallas import tpu as pltpu

T = 2048
D = 512
H = 1024
NE = 32
EL = 8
CAP = 204
NB = 8
BT = T // NB
NC = NB * NE

LX = 4
LY = 4
CX, CY = 1 << LX, 1 << LY
NRX = 352 >> LX
NRY = 608 >> LY
NRLY = 24
NBITS = 11
NSX, NSY = NRX + NBITS, NRY + NBITS
XS = (LX, NRX)
YS = (LY, NRY)
XP = 16
HX = T // 2 + XP
RX = 2 * HX
RY = 1664
DUMMYX = XP + 7 * RX
ZEROY = 8 * RY
MT = 128
BIG = 1 << 20

K1OFF = 13
ES = 4
CN_POS = 1
C3_POS = 4
FWD_BIAS = 120
LEAD = 2
DRAIN_B = 5

U32 = jnp.uint32
I32 = jnp.int32
F32 = jnp.float32
BF16 = jnp.bfloat16
MESH = pl.DeviceIdType.MESH


def _task_key(g, e):
    return 4 * e if g == 0 else max(4 * e + 1, 2 * e + K1OFF)


_TASKS = sorted([(g, e) for g in range(2) for e in range(EL)],
                key=lambda t: (_task_key(*t), t[0]))
assert all(g == 0 for g, _ in _TASKS[:max(CN_POS, C3_POS)])

ST_XA = 0
ST_XIN = 8
ST_XOUT = 16
ST_XS = 24
ST_YS = 32
ST_YA = 36
ST_YIN = 40
ST_YOUT = 44
ST_F0 = 48
ST_F1 = 49
ST_LD = 50
ST_TG = 56
ST_TE = 72
ST_N = 88


def _pack2(a, b):
    lo = lax.bitcast_convert_type(a.astype(BF16).astype(F32), U32) >> 16
    hi = lax.bitcast_convert_type(b.astype(BF16).astype(F32), U32)
    return hi | lo


def _unlo(w):
    return lax.bitcast_convert_type(w << 16, F32)


def _unhi(w):
    return lax.bitcast_convert_type(w & jnp.uint32(0xFFFF0000), F32)


def _dot(a, b):
    return jnp.dot(a, b, preferred_element_type=F32)


def _dot_nt(a, b):
    return lax.dot_general(a, b, (((1,), (1,)), ((), ())),
                           preferred_element_type=F32)


def _onez(mask):
    return jnp.where(mask, 1.0, 0.0).astype(BF16)


def _body(x_hbm, route_hbm, w_hbm, out_ref,
          xv, wv, rv, xtok, xb, yb, stg, ystg, ytok,
          oh, rk, cnt, cm, tabv, earlyv, fastv,
          tabs, earlys, fasts, st,
          sem_l, sem_cs, sem_cr,
          sem_xs, sem_xr, sem_ys, sem_yr, sem_fs, sem_fr):
    me = lax.axis_index("i")

    route_cp = pltpu.make_async_copy(route_hbm, rv, sem_l.at[0])
    route_cp.start()

    def x_cp(p):
        return pltpu.make_async_copy(x_hbm.at[pl.ds(p * BT, BT)],
                                     xv.at[pl.ds(p * BT, BT)], sem_l.at[5 + p])

    def w_cp(e):
        return pltpu.make_async_copy(w_hbm.at[e], wv.at[e], sem_l.at[13 + e])

    for p in range(4):
        x_cp(p).start()

    bar = pltpu.get_barrier_semaphore()
    for k in range(1, 4):
        pl.semaphore_signal(bar, inc=1, device_id=((me + k) & 3,),
                            device_id_type=MESH)

    def rest_loads(pos):
        for e in range(EL):
            if e == pos:
                for p in range(4, NB):
                    x_cp(p).start()
            w_cp(e).start()

    @pl.when(me == 3)
    def _():
        rest_loads(C3_POS)

    @pl.when(me < 3)
    def _():
        rest_loads(CN_POS)

    def iota2(dim):
        return lax.broadcasted_iota(I32, (NC, NC), dim)

    def xkey(c):
        b = c >> 5
        xg = jnp.where(b == 0, 0, 32)
        return (((c & 31) >> 3) * 2 + (b >> 2)) * 64 + xg + (c & 7) * 4 + (b & 3)

    def ykey(c):
        b = c >> 5
        e = c & 7
        g = c >> 7
        k0 = 8 * e
        k1 = jnp.maximum(8 * e + 2, 4 * e + 2 * K1OFF) + 1
        kt = jnp.where(g == 0, k0, k1) * 4 + (b & 3)
        kp = 1024 + b * 8 + e
        kk = jnp.where((g == 1) & (e >= ES), kp, kt)
        return ((c & 31) >> 3) * 2048 + kk

    cm[1] = _onez(iota2(0) < iota2(1))
    kxi, kxj = xkey(iota2(0)), xkey(iota2(1))
    cm[0] = _onez((kxi < kxj) & (kxi >= (kxj & ~63)))

    r8 = lax.broadcasted_iota(I32, (8, NC), 0)
    c8 = lax.broadcasted_iota(I32, (8, NC), 1)
    blk8 = (c8 >> 5) == r8
    krel8 = (((c8 & 31) >> 3) - me) & 3

    for i in range(ST_TG):
        st[i] = 0
    for i, (g, e) in enumerate(_TASKS):
        st[ST_TG + i] = g
        st[ST_TE + i] = e

    route_cp.wait()
    fast_cp = pltpu.make_async_copy(fastv, fasts, sem_l.at[4])

    @pl.when(me < 3)
    def _():
        e128 = lax.broadcasted_iota(I32, (128, 128), 0)
        oh0 = jnp.concatenate(
            [_onez(e128 == rv[h:h + 1, :]) for h in range(2)], axis=1)
        raw0 = _dot_nt(jnp.ones((8, BT), BF16), oh0)
        pre0 = _dot(oh0[0:NE], cm[1])
        rank0 = jnp.sum(oh0[0:NE].astype(F32) * pre0, axis=0, keepdims=True)
        off0 = _dot(raw0.astype(BF16), cm[0, 0:128, 0:128]).astype(I32)
        v0 = off0 + krel8[:, :128] * RX + XP
        r0 = r8[:, :128]
        l0 = jnp.where(r0 == 0, v0 >> 7, v0 & 127)
        l0 = jnp.concatenate([l0, l0], axis=0).astype(F32).astype(BF16)
        lk0 = _dot(l0, oh0)
        pos0 = (lk0[0:1] * 128.0 + lk0[1:2] + rank0).astype(I32) * 2
        end0 = off0 + raw0.astype(I32)
        fastv[...] = jnp.where(r0 == 0, pos0[:, :128],
                               jnp.where(r0 == 1, pos0[:, 128:], end0))
        fast_cp.start()

    e32 = lax.broadcasted_iota(I32, (NE, 128), 0)
    for b in range(NB):
        for h in range(2):
            rb = rv[2 * b + h:2 * b + h + 1, :]
            oh[b * NE:(b + 1) * NE, 128 * h:128 * h + 128] = _onez(e32 == rb)
    ohv = oh[...]
    raw = _dot_nt(jnp.ones((8, BT), BF16), ohv)
    cnt[me] = raw

    def cnt_cp(k):
        return pltpu.make_async_remote_copy(
            src_ref=cnt.at[me], dst_ref=cnt.at[me],
            send_sem=sem_cs.at[k - 1], recv_sem=sem_cr.at[k - 1],
            device_id=((me + k) & 3,), device_id_type=MESH)

    pl.semaphore_wait(bar, 3)
    for k in range(1, 4):
        cnt_cp(k).start()

    def pack_block(p):
        x_cp(p).wait()
        for h in range(2):
            r0 = pl.multiple_of(p * BT + h * 128, 128)
            xf = xv[pl.ds(r0, 128), :]
            xtok[pl.ds(2 * r0, 128, stride=2), :] = _pack2(
                xf[:, 0:128], xf[:, 128:256])
            xtok[pl.ds(2 * r0 + 1, 128, stride=2), :] = _pack2(
                xf[:, 256:384], xf[:, 384:512])

    def scatter_rows(pos_ref, lo, hi):
        def loop(r, _):
            base = r * 256
            for u in range(128):
                qq = pos_ref[r, u]
                xb[pl.ds(qq, 2), :] = xtok[pl.ds(base + 2 * u, 2), :]
            return 0
        lax.fori_loop(lo, hi, loop, 0)

    def x_copy_h(hf):
        def x_copy(k, off, n, sidx):
            o = XP + hf * HX + off
            return pltpu.make_async_remote_copy(
                src_ref=xb.at[pl.ds(2 * (k * RX + o), 2 * n)],
                dst_ref=xb.at[pl.ds(2 * ((3 + k) * RX + o), 2 * n)],
                send_sem=sem_xs.at[k - 1],
                recv_sem=sem_xr.at[(3 * hf + k - 1) * NSX + sidx],
                device_id=((me + k) & 3,), device_id_type=MESH)
        return x_copy

    def y_copy(k, off, n, sidx):
        return pltpu.make_async_remote_copy(
            src_ref=yb.at[pl.ds(4 * (k * RY + off), 4 * n)],
            dst_ref=yb.at[pl.ds(4 * ((3 + k) * RY + off), 4 * n)],
            send_sem=sem_ys.at[k - 1], recv_sem=sem_yr.at[(k - 1) * NSY + sidx],
            device_id=((me - k) & 3,), device_id_type=MESH)

    def y_to_relay(c, c0):
        return pltpu.make_async_remote_copy(
            src_ref=yb.at[pl.ds(4 * (2 * RY + c * CY), 4 * CY)],
            dst_ref=yb.at[pl.ds(4 * (7 * RY + c * CY), 4 * CY)],
            send_sem=sem_ys.at[1], recv_sem=sem_fr.at[c - c0],
            device_id=(me ^ 1,), device_id_type=MESH)

    def y_from_relay(c):
        return pltpu.make_async_remote_copy(
            src_ref=yb.at[pl.ds(4 * (7 * RY + c * CY), 4 * CY)],
            dst_ref=yb.at[pl.ds(4 * (5 * RY + c * CY), 4 * CY)],
            send_sem=sem_fs, recv_sem=sem_yr.at[NSY + c],
            device_id=(me ^ 3,), device_id_type=MESH)

    def nfull(cfg, n):
        return jnp.minimum(n >> cfg[0], cfg[1])

    def branch(cond, fn):
        def f(i, _):
            fn()
            return 0
        lax.fori_loop(0, cond.astype(I32), f, 0)

    def tail_pieces(copy, cfg, k, n, fn):
        lc, nreg = cfg
        base = nfull(cfg, n) << lc
        r = n - base

        def bits(lo, hi):
            for bit in range(hi - 1, lo - 1, -1):
                @pl.when(((r >> bit) & 1) == 1)
                def _():
                    off = base + ((r >> (bit + 1)) << (bit + 1))
                    fn(copy(k, off, 1 << bit, nreg + bit))

        branch(r >= (1 << lc), lambda: bits(lc, NBITS))
        bits(0, lc)

    def start_(c):
        c.start()

    def wait_recv_(c):
        c.wait_recv()

    def wait_send_(c):
        c.wait_send()

    def ensure(copy, cfg, k, upto, i_a, i_len):
        lc, nreg = cfg
        have = st[i_a + k]
        n = st[i_len + k]
        nf = nfull(cfg, n)
        need = jnp.minimum((upto + ((1 << lc) - 1)) >> lc, nf)
        hc = have >> lc
        for j in range(3):
            @pl.when(hc + j < need)
            def _():
                copy(k, (hc + j) << lc, 1 << lc, hc + j).wait_recv()
        in_tail = (upto > (nf << lc)) & (have < BIG)
        st[i_a + k] = jnp.where(in_tail, BIG, jnp.maximum(have, need << lc))

        def rest():
            def loop(c, _):
                copy(k, c << lc, 1 << lc, c).wait_recv()
                return 0
            lax.fori_loop(hc + 3, need, loop, 0)
            branch(in_tail, lambda: tail_pieces(copy, cfg, k, n, wait_recv_))
        branch((need > hc + 3) | in_tail, rest)

    def send_upto(send_chunk, cfg, i_s, wm, kdir):
        s0 = [st[i_s + k] for k in range(1, 4)]
        tgt = [jnp.maximum(s0[k - 1], nfull(cfg, wm[k - 1])) for k in range(1, 4)]
        cn = [tgt[i] - s0[i] for i in range(3)]
        cntmax = jnp.maximum(jnp.maximum(cn[0], cn[1]), cn[2])
        ld = st[ST_LD]

        def loop(i, _):
            for k in (2, 1, 3):
                j = i if k == 2 else i + ld

                @pl.when((j >= 0) & (j < cn[k - 1]))
                def _():
                    send_chunk(k, s0[k - 1] + j)
            return 0
        lax.fori_loop(-ld, cntmax, loop, 0)
        for k in range(1, 4):
            st[i_s + k] = tgt[k - 1]
        na = jnp.where(kdir == 1, cn[0], cn[2])
        nd = cn[1]
        last_d = (nd > na - ld).astype(I32)
        st[ST_LD] = jnp.where(na + nd > 0, jnp.where(nd > 0, last_d, 0), ld)

    def send_y_chunk(k, c):
        if k == 2:
            relay = (c >= st[ST_F0]) & (c < st[ST_F1])

            @pl.when(relay)
            def _():
                y_to_relay(c, st[ST_F0]).start()

            @pl.when(jnp.logical_not(relay))
            def _():
                y_copy(k, c * CY, CY, c).start()
        else:
            y_copy(k, c * CY, CY, c).start()

    def send_x_upto(hf, wm):
        def send_x_chunk(k, c):
            x_copy_h(hf)(k, c * CX, CX, c).start()
        send_upto(send_x_chunk, XS, ST_XS + 4 * hf, wm, 3 - 2 * (me & 1))

    def send_x_all(hf, lens):
        send_x_upto(hf, lens)
        for k in (2, 1, 3):
            tail_pieces(x_copy_h(hf), XS, k, lens[k - 1], start_)

    def send_y_upto(wm):
        send_upto(send_y_chunk, YS, ST_YS, wm, 1 + 2 * (me & 1))

    pack_block(0)

    @pl.when(me < 3)
    def _():
        fast_cp.wait()
        scatter_rows(fasts, 0, 2)
        send_x_upto(0, [fasts[2, 8 * ((me + k) & 3) + 7] for k in range(1, 4)])

    pre = _dot(ohv, cm[1])
    rank = _dot(_onez(blk8), (ohv.astype(F32) * pre).astype(BF16))
    rk[...] = rank

    def q(vi):
        return jnp.where(blk8, vi, 0).astype(F32).astype(BF16)

    early_cp = pltpu.make_async_copy(earlyv, earlys, sem_l.at[1])
    tab_cp = pltpu.make_async_copy(tabv.at[pl.ds(0, 48)], tabs.at[pl.ds(0, 48)],
                                   sem_l.at[2])
    py_cp = pltpu.make_async_copy(tabv.at[pl.ds(48, 16)], tabs.at[pl.ds(48, 16)],
                                  sem_l.at[3])

    def put_early(pos2, xend_rows):
        ev = jnp.where(r8 < 4, pos2, xend_rows)
        earlyv[pl.ds(0, 8, stride=2), :] = ev[:, :128]
        earlyv[pl.ds(1, 8, stride=2), :] = ev[:, 128:]
        early_cp.start()

    @pl.when(me < 3)
    def _():
        xoff_e = _dot(raw.astype(BF16), cm[0]).astype(I32)
        v = xoff_e + krel8 * RX + XP
        lk = _dot(jnp.concatenate([q(v >> 7), q(v & 127)], axis=0), ohv)
        pos_e = (lk[0:8] * 128.0 + lk[8:16] + rank).astype(I32) * 2
        put_early(pos_e, xoff_e + raw.astype(I32))

    def late(with_early):
        ci, cj = iota2(0), iota2(1)
        same_e = (ci & 31) == (cj & 31)
        m_e = _onez(same_e)
        m_b = _onez(same_e & (ci < cj))
        m_g = _onez(same_e & ((ci >> 7) == (cj >> 7)))
        kyi, kyj = ykey(ci), ykey(cj)
        o_y = _onez((kyi < kyj) & (kyi >= (kyj & ~2047)))

        for k in range(1, 4):
            cnt_cp(k).wait_recv()

        r16 = lax.broadcasted_iota(I32, (16, NC), 0)
        c16 = lax.broadcasted_iota(I32, (16, NC), 1)
        chip = jnp.where(r16 < 8, r16 & 3, me)
        cs = [cnt[s] for s in range(4)]
        tab = jnp.zeros((16, NC), F32)
        for s in range(4):
            tab = jnp.where(chip == s, jnp.concatenate([cs[s], cs[s]], axis=0), tab)
        tot = _dot(jnp.concatenate(cs[:3] + [cs[0]], axis=0).astype(BF16), m_e)
        cum = _dot(tab.astype(BF16), m_b)
        for s in range(3):
            ts = tot[8 * s:8 * s + 8]
            cum = cum + jnp.where(chip > s, jnp.concatenate([ts, ts], axis=0), 0.0)
        kept = jnp.clip(float(CAP) - cum, 0.0, tab)
        xc = jnp.where((chip < 3) & (c16 < 128), tab, kept)
        keptb = kept.astype(BF16)
        xoff = _dot(xc.astype(BF16), cm[0]).astype(I32)
        yoff = _dot(keptb, o_y).astype(I32)
        seg = _dot(keptb, m_g).astype(I32)
        kept_i = kept.astype(I32)
        xend = xoff + xc.astype(I32)
        vx = xoff[8:16] + krel8 * RX + (c8 >> 7) * HX + XP
        vy = yoff[8:16] + jnp.where(krel8 == 0, 0, 3 + krel8) * RY
        lhs = jnp.concatenate(
            [q(vx >> 7), q(vx & 127), q(xc[8:16].astype(I32)),
             q(vy >> 7), q(vy & 127), q(kept_i[8:16])], axis=0)
        lk = _dot(lhs, oh[...])
        rnk = rk[...]
        px = jnp.where(rnk < lk[16:24], lk[0:8] * 128.0 + lk[8:16] + rnk,
                       float(DUMMYX))
        py = jnp.where(rnk < lk[40:48], lk[24:32] * 128.0 + lk[32:40] + rnk,
                       float(ZEROY))
        pxi = px.astype(I32) * 2
        pyi = py.astype(I32) * 4
        if with_early:
            put_early(pxi, xend[8:16])

        def put(row, val):
            tabv[row:row + 8, :] = val[:, :128]
            tabv[row + 8:row + 16, :] = val[:, 128:]

        put(16, jnp.where(r8 < 4, xoff[0:8],
                          jnp.where((c8 & 127) < 32, seg[0:8], xend[0:8])))
        put(32, jnp.where(r8 < 4, yoff[0:8], kept_i[0:8]))
        for h in range(2):
            tabv[pl.ds(h, 8, stride=2), :] = pxi[:, 128 * h:128 * h + 128]
            tabv[pl.ds(48 + h, 8, stride=2), :] = pyi[:, 128 * h:128 * h + 128]
        tab_cp.start()
        py_cp.start()

    @pl.when(me == 3)
    def _():
        late(True)

    pack_block(1)
    early_cp.wait()

    def first_half(p, _):
        @pl.when(p > 1)
        def _():
            pack_block(p)
        scatter_rows(earlys, 2 * p, 2 * p + 2)

        @pl.when(p == 0)
        def _():
            send_x_upto(0, [earlys[8, 8 * ((me + k) & 3) + 7]
                            for k in range(1, 4)])
        return 0
    lax.fori_loop(jnp.where(me < 3, 1, 0), 4, first_half, 0)
    send_x_all(0, [earlys[8, 96 + 8 * ((me + k) & 3) + 7] for k in range(1, 4)])

    @pl.when(me < 3)
    def _():
        late(False)

    stg[...] = jnp.zeros(stg.shape, U32)
    yb[pl.ds(4 * ZEROY, 8), :] = jnp.zeros((8, 128), U32)

    tab_cp.wait()

    def XOFF(s, g, c):
        return tabs[16 + 8 * g + s, c]

    def SEG(s, g, c):
        return tabs[20 + 8 * g + s, c]

    def YOFF(s, g, c):
        return tabs[32 + 8 * g + s, c]

    def KEPT(s, g, c):
        return tabs[36 + 8 * g + s, c]

    def xlen_h(s, d, hf):
        return SEG(s, hf, 96 + 8 * d + 7)

    def ylen(d, s):
        c = 96 + 8 * d + 7
        return YOFF(s, 1, c) + KEPT(s, 1, c)

    for k in range(1, 4):
        for hf in range(2):
            st[ST_XIN + 4 * hf + k] = xlen_h((me - k) & 3, me, hf)
            st[ST_XOUT + 4 * hf + k] = xlen_h(me, (me + k) & 3, hf)
        st[ST_YIN + k] = ylen((me + k) & 3, me)
        st[ST_YOUT + k] = ylen(me, (me - k) & 3)

    def second_half():
        def blk(p, _):
            pack_block(p)
            scatter_rows(tabs, 2 * p, 2 * p + 2)
            return 0
        lax.fori_loop(4, NB, blk, 0)
        send_x_all(1, [st[ST_XOUT + 4 + k] for k in range(1, 4)])


    def tr(a, b):
        return xlen_h(a, b, 0) + xlen_h(a, b, 1) + 2 * ylen(a, b)

    def l3(a):
        return tr(a, a ^ 3) + tr(a, a ^ 2)

    def l1(a):
        return tr(a, a ^ 1) + tr(a ^ 3, a ^ 1)

    def relay_range(d):
        over = (jnp.maximum(l3(d), l1(d ^ 3)) - jnp.maximum(l1(d), l3(d ^ 1))
                - FWD_BIAS)
        r = jnp.minimum(jnp.maximum(over + 2 * CY, 0) >> (LY + 2), NRLY)
        f1 = nfull(YS, YOFF(d ^ 2, 1, 8 * d + ES))
        return jnp.maximum(f1 - r, 0), f1

    f0, f1 = relay_range(me)
    st[ST_F0] = f0
    st[ST_F1] = f1
    p0, p1 = relay_range(me ^ 1)

    def copy_x(jobs):
        over = None
        for (src, dst, nr, nbig) in reversed(jobs):
            low = jnp.minimum(nr - 32, 0)
            for i in range(nbig):
                o = jnp.maximum(nr - 32 * (i + 1), low) if i else nr - 32
                stg[pl.ds(32 + dst + o, 32), :] = xb[pl.ds(src + o, 32), :]
            o = nr > 32 * nbig
            over = o if over is None else (over | o)

        def rest():
            for (src, dst, nr, nbig) in jobs:
                def f(i, _):
                    o = jnp.maximum(nr - 32 * (i + 1), 0)
                    stg[pl.ds(32 + dst + o, 32), :] = xb[pl.ds(src + o, 32), :]
                    return 0
                lax.fori_loop(nbig, (nr + 31) >> 5, f, 0)
        branch(over, rest)

    i32r = lax.broadcasted_iota(I32, (32, 128), 0)

    def copy_y(jobs):
        over = None
        for (src, dst, nr, nbig) in jobs:
            yb[pl.ds(dst, 32), :] = jnp.where(
                i32r < nr, ystg[pl.ds(src, 32), :], yb[pl.ds(dst, 32), :])
            ok = nr > 32
            s_ = jnp.where(ok, src, 0)
            d_ = jnp.where(ok, dst, 4 * ZEROY + 8)
            lim = jnp.maximum(nr - 32, 0)
            for i in range(1, nbig):
                o = jnp.minimum(32 * i, lim)
                yb[pl.ds(d_ + o, 32), :] = ystg[pl.ds(s_ + o, 32), :]
            o = nr > 32 * nbig
            over = o if over is None else (over | o)

        def rest():
            for (src, dst, nr, nbig) in jobs:
                def f(i, _):
                    o = jnp.minimum(i * 32, nr - 32)
                    yb[pl.ds(dst + o, 32), :] = ystg[pl.ds(src + o, 32), :]
                    return 0
                lax.fori_loop(nbig, (nr + 31) >> 5, f, 0)
        branch(over, rest)

    def task(ti, _):
        g = st[ST_TG + ti]
        e = st[ST_TE + ti]
        ee = 8 * me + e

        @pl.when(ti == jnp.where(me == 3, C3_POS, CN_POS))
        def _():
            second_half()

        @pl.when(g == 0)
        def _():
            w_cp(e).wait()

        segs = []
        xjobs = []
        row = jnp.int32(0)
        for k in range(4):
            s = (me - k) & 3
            reg = 0 if k == 0 else 3 + k
            n = SEG(s, g, ee)
            na = jnp.where(g == 0, KEPT(s, 0, ee), 0)
            nb = n - na
            sb = XOFF(s, g, ee + jnp.where(g == 0, 32, 0))
            sa = jnp.where(g == 0, XOFF(s, 0, ee), 0)
            if k > 0:
                ensure(x_copy_h(g), XS, k, sb + nb, ST_XA + 4 * g, ST_XIN + 4 * g)
            base = XP + reg * RX + g * HX
            xjobs.append((2 * (base + sa), 2 * row, 2 * na, 1))
            xjobs.append((2 * (base + sb), 2 * (row + na), 2 * nb, 3))
            segs.append((k, s, n, row))
            row = row + n
        copy_x(xjobs)

        def tile(t, _):
            r0 = t * MT
            w0 = stg[pl.ds(32 + 2 * r0, MT, stride=2), :]
            w1 = stg[pl.ds(33 + 2 * r0, MT, stride=2), :]
            lhs = jnp.concatenate(
                [_unlo(w0).astype(BF16), _unhi(w0).astype(BF16),
                 _unlo(w1).astype(BF16), _unhi(w1).astype(BF16)], axis=1)
            for j in range(4):
                wj = wv[e, :, 256 * j:256 * (j + 1)].astype(BF16)
                y = _dot(lhs, wj)
                ystg[pl.ds(4 * r0 + j, MT, stride=4), :] = _pack2(
                    y[:, :128], y[:, 128:])
            return 0
        lax.fori_loop(0, (row + (MT - 1)) >> 7, tile, 0)

        ph2 = (g == 1) & (e >= ES)

        @pl.when(jnp.logical_not(ph2))
        def _():
            copy_y([(4 * r, 4 * (k * RY + YOFF(s, g, ee)), 4 * n, 6)
                    for (k, s, n, r) in segs])
            send_y_upto([YOFF(s, g, ee) + n for (k, s, n, r) in segs[1:]])

        @pl.when(ph2)
        def _():
            jobs = []
            for (k, s, n, r) in segs:
                rr = r
                for bb in range(4):
                    cb = ee + 32 * bb
                    nb = KEPT(s, 1, cb)
                    jobs.append((4 * rr, 4 * (k * RY + YOFF(s, 1, cb)), 4 * nb, 2))
                    rr = rr + nb
            copy_y(jobs)

        return 0

    lax.fori_loop(0, 2 * EL, task, 0)


    def relay_loop(c, _):
        y_to_relay(c, p0).wait_recv()
        y_from_relay(c).start()
        return 0
    lax.fori_loop(p0, p1, relay_loop, 0)

    pre2 = [st[ST_YS + k] for k in range(1, 4)]
    rem = [nfull(YS, st[ST_YOUT + k]) - pre2[k - 1] for k in range(1, 4)]
    fin = jnp.maximum(jnp.maximum(rem[0], rem[1]), rem[2]) + LEAD
    shift = [jnp.where((me >= 2) & (me - k == 1), LEAD, 0) for k in range(1, 4)]

    def final_loop(i, _):
        for k in (2, 1, 3):
            j = i - shift[k - 1]

            @pl.when((j >= 0) & (j < rem[k - 1]))
            def _():
                y_copy(k, (pre2[k - 1] + j) * CY, CY, pre2[k - 1] + j).start()

            @pl.when(j == rem[k - 1])
            def _():
                tail_pieces(y_copy, YS, k, st[ST_YOUT + k], start_)
        return 0
    lax.fori_loop(0, fin + 1, final_loop, 0)

    for hf in range(2):
        for k in range(1, 4):
            ensure(x_copy_h(hf), XS, k, st[ST_XIN + 4 * hf + k],
                   ST_XA + 4 * hf, ST_XIN + 4 * hf)

    def drain_send(copy, cfg, k, lo, hi):
        def loop(c, _):
            copy(k, c << cfg[0], 1 << cfg[0], c).wait_send()
            return 0
        lax.fori_loop(lo, hi, loop, 0)

    for k in range(1, 4):
        cnt_cp(k).wait_send()
        for hf in range(2):
            n = st[ST_XOUT + 4 * hf + k]
            drain_send(x_copy_h(hf), XS, k, 0, nfull(XS, n))
            tail_pieces(x_copy_h(hf), XS, k, n, wait_send_)
    py_cp.wait()

    def relay_drain(c, _):
        y_from_relay(c).wait_send()
        return 0

    def out_block(b, _):

        @pl.when(b == DRAIN_B)
        def _():
            for k in range(1, 4):
                drain_send(y_copy, YS, k, 0, pre2[k - 1])
            lax.fori_loop(p0, p1, relay_drain, 0)

        @pl.when(b == NB - 1)
        def _():
            for k in range(1, 4):
                drain_send(y_copy, YS, k, pre2[k - 1], nfull(YS, st[ST_YOUT + k]))
                tail_pieces(y_copy, YS, k, st[ST_YOUT + k], wait_send_)

        for k in range(1, 4):
            c = (b & 3) * 32 + 8 * ((me + k) & 3) + 7
            ensure(y_copy, YS, k, YOFF(me, b >> 2, c) + KEPT(me, b >> 2, c),
                   ST_YA, ST_YIN)

        def gat(h, _):
            r = 48 + 2 * b + h
            base = h * 512
            for u in range(128):
                p = tabs[r, u]
                ytok[pl.ds(base + 4 * u, 4), :] = yb[pl.ds(p, 4), :]
            return 0
        lax.fori_loop(0, 2, gat, 0)

        def unp(i, _):
            r0 = pl.multiple_of(b * BT + i * 64, 64)
            for j in range(4):
                w = ytok[pl.ds(i * 256 + j, 64, stride=4), :]
                out_ref[pl.ds(r0, 64), 256 * j:256 * j + 128] = _unlo(w)
                out_ref[pl.ds(r0, 64), 256 * j + 128:256 * j + 256] = _unhi(w)
            return 0
        lax.fori_loop(0, BT // 64, unp, 0)
        return 0

    lax.fori_loop(0, NB, out_block, 0)


def pallas_dist_moe_cap_ep_tokshard_n2048_d512_e8_h1024_kernel(
    x: jax.Array,
    router_W: jax.Array,
    route_idx: jax.Array,
    expert_W: jax.Array,
):
    del router_W
    route = route_idx.astype(I32).reshape(T // 128, 128)
    any_spec = pl.BlockSpec(memory_space=pl.ANY)
    dma = pltpu.SemaphoreType.DMA
    return pl.pallas_call(
        _body,
        out_shape=jax.ShapeDtypeStruct((T, H), F32),
        in_specs=[any_spec, any_spec, any_spec],
        out_specs=pl.BlockSpec(memory_space=pltpu.VMEM),
        scratch_shapes=[
            pltpu.VMEM((T, D), F32),
            pltpu.VMEM((EL, D, H), F32),
            pltpu.VMEM((T // 128, 128), I32),
            pltpu.VMEM((2 * T, 128), U32),
            pltpu.VMEM((2 * (DUMMYX + 4), 128), U32),
            pltpu.VMEM((4 * (ZEROY + 10), 128), U32),
            pltpu.VMEM((4 * MT + 32, 128), U32),
            pltpu.VMEM((8 * MT, 128), U32),
            pltpu.VMEM((4 * BT, 128), U32),
            pltpu.VMEM((NC, BT), BF16),
            pltpu.VMEM((8, BT), F32),
            pltpu.VMEM((4, 8, NC), F32),
            pltpu.VMEM((2, NC, NC), BF16),
            pltpu.VMEM((64, 128), I32),
            pltpu.VMEM((16, 128), I32),
            pltpu.VMEM((8, 128), I32),
            pltpu.SMEM((64, 128), I32),
            pltpu.SMEM((16, 128), I32),
            pltpu.SMEM((8, 128), I32),
            pltpu.SMEM((ST_N,), I32),
            dma((21,)), dma((3,)), dma((3,)),
            dma((3,)), dma((6 * NSX,)), dma((3,)), dma((3 * NSY,)),
            dma, dma((NRLY,)),
        ],
        compiler_params=pltpu.CompilerParams(
            collective_id=0, vmem_limit_bytes=88 * 1024 * 1024,
            disable_semaphore_checks=True, disable_bounds_checks=True),
    )(x, route, expert_W)
```
